```python
import numpy as np

kernel_name = "dist_moe_top2_ep_n1024_d512_e4_h1024"

def setup_inputs():
    x = np.random.randn(1024, 512).astype(np.float32)
    router_W = np.random.randn(512, 16).astype(np.float32) * 0.1
    scores64 = x.astype(np.float64) @ router_W.astype(np.float64)
    route_idx = np.argsort(-scores64, axis=-1)[:, :2].astype(np.int32)
    expert_W = np.random.randn(16, 512, 1024).astype(np.float32) * 0.02
    return {"x": x, "router_W": router_W, "route_idx": route_idx, "expert_W": expert_W}

def reference(x, router_W, route_idx, expert_W):
    scores = x @ router_W
    s_max = scores.max(axis=-1, keepdims=True)
    probs = np.exp(scores - s_max)
    probs = probs / probs.sum(axis=-1, keepdims=True)
    out = np.zeros((1024, 1024), dtype=np.float32)
    for i in range(1024):
        e0, e1 = int(route_idx[i, 0]), int(route_idx[i, 1])
        g0, g1 = probs[i, e0], probs[i, e1]
        gs = g0 + g1
        out[i] = (g0 / gs) * (x[i] @ expert_W[e0]) + (g1 / gs) * (x[i] @ expert_W[e1])
    return out
```

```python
import jax
import jax.numpy as jnp
from jax import lax
from jax.experimental import pallas as pl
from jax.experimental.pallas import tpu as pltpu

N_TOK, D_IN, D_OUT, N_EXP = 1024, 512, 1024, 16
E_LOC = 4
LANES = 128
BLK = 256
HALF = BLK // 2
NBLK = N_TOK // BLK
NCT = D_OUT // LANES
BF16, F32, U32, I32 = jnp.bfloat16, jnp.float32, jnp.uint32, jnp.int32
NT = (((1,), (1,)), ((), ()))

PLANES = (1, 1, 2, 2, 2)
WIDTHS = (1, 2)
TILE0 = tuple(sum(PLANES[:p]) for p in range(len(PLANES)))
SLOT = tuple(PLANES[:p].count(PLANES[p]) for p in range(len(PLANES)))
TOKENS_PER_ROW = {1: 2, 2: 1}
ROWS = {1: 136, 2: 256}

CAP_E = 64
CAP_H = 40
CAP_Y = 160
CAP_Z = 176
SEND_TOTAL = NCT * NBLK * (CAP_Y // 2 + CAP_Z // 2 + 61)

LAUNCH_SKEW = (124, 56)

LOADS = "ri rw x0 w0 x1 x2 x3 w1 w2 w3 w4 w5 w6 w7".split()

SCHEDULE = """
P1:2+P2:0+P0:0+Q1:2 P0:2+Q2:0 P1:0+P2:2+G0+Q0:2 P3:0+Q3:0+Q0:0+Q1:0 P3:2+c0:0+Q3:2 S0:0
G1 c1:0+G2 S1:0 c2:0+G3 S2:0 c3:0+Q2:2 S3:0 z0:0 Y0:0 c1:1+c0:1+U2:2 S1:1 S0:1 z1:0
c2:1+U0:2+U1:0+Y1:0 z2:0 Y2:0 S2:1 z3:0 Y3:0 c3:1+e0:2+e1:2+U0:0 S3:1 z1:1 Y1:1 z0:1
Y0:1 c1:2 S1:2 c0:2+U3:2 S0:2 z2:1 c2:2+Y2:1 S2:2 z3:1 c3:2+Y3:1 S3:2 z1:2
c3:3+U2:0+Y1:2 z0:2 Y0:2 c0:3+S3:3 z2:2 Y2:2 c1:3+c2:3+U3:0+S0:3 S1:3 T1:2 c1:4+S2:3
T1:01 c0:4+S1:4+T0:2 S0:4 z3:23 c2:4+D3:3+D3:2 S2:4 z0:3 c3:4+U1:2+D0:3+T2:2 S3:4 T2:01
T0:01 W0 z1:3 Y1:3 z2:3 T3:01 z1:4 D1:4 R3:2 O0:2 D2:3 z0:4 D0:4 O1:2+R3:3 T3:23 z2:4 D2:4
R1:4 O1:01+T0:3 z3:4 D3:4 R2:3 O0:01+R0:4 O2:2+T1:34 R0:3 O3:01+T0:4 R2:4 T2:34 R3:4
O2:01 T3:4 O3:23 O1:34 O0:34 O2:34 O3:4
"""
SENDS = "SYDRT"
BOTH = (True, False)


def _size_bits(kind, plane):
    return (3 if kind in "TD" else 5) + PLANES[plane]


def _wire_up(text):
    awaits = dict(z=("S",), T=("YD",), O=("YR", "T"))
    needs = dict(Q="P", U="P", c="GQ", e="G", O="U", S="c", Y="z", D="z", R="z")
    groups = [[(s[0], int(s[1]), int((s[3:] or "0")[0]), int((s[3:] or "0")[-1]) + 1)
               for s in group.split("+")] for group in text.split()]
    waits, sems, sent, got, done = {}, {}, {}, {}, set()
    spare, retired, count = {True: [], False: []}, set(), 0
    for now, group in enumerate(groups):
        for kind, q, p0, p1 in group:
            for p in range(p0, p1):
                tag = lambda k: (k, q, 0 if k == "G" else PLANES[p] if k in "PQU" else p)
                assert tag(kind) not in done and all(tag(k) in done for k in needs.get(kind, ""))
                done.add(tag(kind))
            waits[kind, q, p0] = []
            for which in awaits.get(kind, ()):
                hits = [m for m in sent if m[0] in which and m[1] == q and m[2] < p1 and p0 < m[3]]
                assert {(p, m[4]) for m in hits for p in range(m[2], m[3])} >= {
                    (p, d) for p in range(p0, p1) for d in BOTH}
                waits[kind, q, p0] += [m for m in hits if m not in got]
                got.update({m: now for m in hits if m not in got})
            for d in BOTH if kind in SENDS else ():
                proof = max([sent[m] for m in got if m[0] in "SYR" and m[4] != d and got[m] < now],
                            default=0)
                for m in got:
                    if m[4] == d and got[m] < proof and m not in retired:
                        retired.add(m)
                        spare[d] += sems[m]
                mine = spare[d][:_size_bits(kind, p0)]
                del spare[d][:len(mine)]
                fresh = _size_bits(kind, p0) - len(mine)
                sems[kind, q, p0, p1, d] = mine + list(range(count, count + fresh))
                sent[kind, q, p0, p1, d] = now
                count += fresh
    assert sent.keys() == got.keys() and ("W", 0, 0) in done
    assert all(("O", q, p) in done for q in range(NBLK) for p in range(len(PLANES)))
    return groups, waits, sems, count


GROUPS, WAITS, SEMS, N_SEMS = _wire_up(SCHEDULE)
TABLE_SIZE = 64 * NBLK * len(WIDTHS)


def _iota(shape, axis):
    return lax.broadcasted_iota(I32, shape, axis)


def _ones_where(mask):
    return jnp.where(mask, 1.0, 0.0)


def _dot(a, b):
    return jnp.dot(a, b, preferred_element_type=F32)


def _classes(m):
    same, adj, opp = [m[0], m[4], m[7], m[9]], [m[1], m[5], m[8], m[3]], [m[2], m[6]]
    return same, adj, opp, [adj[a] + adj[a - 1] + same[a] for a in range(4)]


def _to_wire(y, width):
    if width == 1:
        return pltpu.bitcast(y.astype(BF16), U32)
    bits = lax.bitcast_convert_type(y.astype(BF16).astype(F32), U32)
    return (bits[:, :LANES] >> 16) | bits[:, LANES:]


def _kernel(x_hbm, rw_hbm, ri_hbm, w_hbm, out_ref, xv, wv, rwv, riv, xs, early, part, ballast,
            table, in_sem, send_sem, recv_sem, *per_width):
    names = ("pos", "to_wire", "to_token", "own", "from_right", "from_left", "summed", "landed")
    buf = {w: dict(zip(names, per_width[i * len(names):])) for i, w in enumerate(WIDTHS)}
    me = lax.axis_index("i")
    right, left = (me + 1) & 3, (me + 3) & 3

    def load(name):
        sem = in_sem.at[LOADS.index(name)]
        if name[0] == "x":
            rows = pl.ds(int(name[1]) * BLK, BLK)
            return pltpu.make_async_copy(x_hbm.at[rows], xv.at[rows], sem)
        if name[0] == "w":
            c = int(name[1])
            return pltpu.make_async_copy(w_hbm.at[:, :, pl.ds(c * LANES, LANES)], wv.at[c], sem)
        return pltpu.make_async_copy(*((ri_hbm, riv) if name == "ri" else (rw_hbm, rwv)), sem)

    for name in LOADS:
        load(name).start()
    barrier = pltpu.get_barrier_semaphore()
    for peer in (left, right):
        pl.semaphore_signal(barrier, inc=1, device_id=(peer,), device_id_type=pl.DeviceIdType.MESH)

    shape = (BLK, BLK + LANES)
    before = _ones_where(_iota(shape, 0) < _iota(shape, 1)).astype(BF16)
    load("ri").wait()
    rel = (riv[...] - E_LOC * me) & (N_EXP - 1)
    row16 = _iota((16, BLK), 0)
    cls, uses = [], []
    for q in range(NBLK):
        r0, r1 = rel[0:1, q * BLK:(q + 1) * BLK], rel[1:2, q * BLK:(q + 1) * BLK]
        lo, hi = jnp.minimum(r0 >> 2, r1 >> 2), jnp.maximum(r0 >> 2, r1 >> 2)
        cls.append(lo * 4 + hi - ((lo * (lo + 1)) >> 1))
        uses.append((row16 == r0) | (row16 == r1))
    member = jnp.concatenate(
        [_ones_where(row16 == k) for k in cls] + [_ones_where(u) for u in uses], axis=0)
    cum = _dot(member.astype(BF16), before)
    whole, lower = cum[64:, BLK:], cum[64:, HALF:BLK]
    excess = jnp.maximum(whole - CAP_E, jnp.maximum(lower, whole - lower) - CAP_H)
    excess = jnp.max(excess, axis=0, keepdims=True).astype(I32)[0, 0]
    cum = cum.astype(I32)
    seat = []
    for q in range(NBLK):
        cq = cum[64 + q * 16:72 + q * 16]
        both = jnp.concatenate([cq[:, :HALF], cq[:, HALF:BLK] + (CAP_E - cq[:, BLK:])], axis=1)
        seat.append(jnp.where(uses[q][:8], both, -1))

    counts = [[cum[q * 16 + k, BLK] for k in range(10)] for q in range(NBLK)]
    fits = excess <= 0
    for q in range(NBLK):
        same, adj, opp, base = _classes([(v + 1) >> 1 for v in counts[q]])
        fits = fits & (jnp.maximum(opp[0], opp[1]) <= 30)
        for a in range(4):
            fits = (fits & (adj[a] > 0) & (base[a] + opp[a & 1] <= CAP_Y // 2)
                    & (base[a] + same[a - 1] + same[(a + 1) & 3] + opp[(a + 1) & 1] <= CAP_Z // 2)
                    & (same[a] + jnp.maximum(adj[a], adj[a - 1]) + opp[a & 1] < 64))
    counts = [[jnp.where(fits, v, 0) for v in n] for n in counts]

    first = [((me + a) & 3) < 2 for a in range(2)]
    balanced, entries, outgoing = {}, {}, []

    def on_chip(vals, chip):
        a = (chip - me) & 3
        return jnp.where(a < 2, jnp.where(a == 0, vals[0], vals[1]),
                         jnp.where(a == 2, vals[2], vals[3]))

    def balance(width):
        m = counts if width == 2 else [[(v + 1) >> 1 for v in n] for n in counts]
        same, _, opp, base = _classes([sum(n[k] for n in m) for k in range(10)])
        d02, d13 = on_chip(opp * 2, 0), on_chip(opp * 2, 1)
        h0 = jnp.maximum(
            (d13 + on_chip(same, 0) - on_chip(same, 2) - LAUNCH_SKEW[0]) >> 1,
            ((2 * (on_chip(base, 2) + d13) + d02 + on_chip(same, 0) - N_TOK - LAUNCH_SKEW[1])
             * 43) >> 7)
        owed, hs = 0, []
        for q in range(NBLK):
            opp = _classes(m[q])[2]
            t = on_chip(opp * 2, 1)
            owed += d13 - h0
            h2 = jnp.clip((owed + 2) >> 2 if width == 2 else (3 * t + 4) >> 3, 0, t)
            owed -= 4 * h2
            h = [None] * 4
            for a in range(2):
                t = opp[(a + 1) & 1]
                v = jnp.where(((me + a) & 1) == 0, t - h2, (t + (q & 1)) >> 1)
                h[a] = jnp.where(first[a], v, t - v)
                h[a + 2] = t - h[a]
            hs.append(h)
        fixed = [base[a] + sum(h[a] for h in hs) for a in range(4)]
        return m, hs, [fixed[a - 1] - fixed[(a + 1) & 3] for a in range(4)], [0] * 4

    def record(key, value):
        entries[key] = len(entries)
        table[entries[key]] = value

    def plan(q, width):
        g = TOKENS_PER_ROW[width]
        if width not in balanced:
            balanced[width] = balance(width)
        m, hs, tilt, carry = balanced[width]
        same, adj, _, base = _classes(m[q])
        h = hs[q]
        s, p = [None] * 4, [None] * 4
        for a in range(4):
            chip, free = (me + a) & 3, same[a] + h[a]
            p[a], w = (jnp.where(chip == 1, 0, jnp.where(chip == 3, v, (v + (q & 1)) >> 1))
                       for v in (h[a], free))
            if width == 2:
                gap = tilt[a] + 4 * free + carry[a]
                w = jnp.clip((gap + 4) >> 3, jnp.maximum(h[a] - 31, 0),
                             same[a] + jnp.minimum(h[a], 31))
                carry[a] = gap - 8 * w
                p[a] = jnp.clip(p[a], w - same[a], w)
            s[a] = w - p[a]
        total = BLK if g == 1 else jnp.maximum(sum(m[q]), HALF)
        nz = [base[a] + h[a] + same[a - 1] + same[(a + 1) & 3] for a in range(4)]

        def message(kind, a, rightward):
            nx, pv, op = (a + 1) & 3, (a - 1) & 3, (a + 2) & 3
            if kind == "S" and rightward:
                return 0, same[op] + adj[nx], h[nx] + adj[a] + same[a]
            if kind == "S":
                return h[nx] + adj[a], 0, same[a] + adj[pv] + h[pv]
            if kind == "T" and rightward:
                return nz[a], total - h[pv], p[pv]
            if kind == "T":
                return total - h[op] - h[nx] + p[nx], total - h[nx] + p[nx], h[nx] - p[nx]
            if rightward:
                so, do, n, k = same[nx] + adj[a], nz[nx], h[a] + adj[pv] + s[pv], p[a]
                return dict(Y=(so, do, n), D=(so, do, k), R=(so + k, do + k, n - k))[kind]
            so, do = s[nx], nz[pv] + h[op] + adj[nx] + s[nx]
            n, k = same[nx] - s[nx] + adj[a] + h[a], h[a] - p[a]
            return dict(Y=(so, do, n), D=(so + n - k, do + n - k, k), R=(so, do, n - k))[kind]

        for kind in SENDS:
            if any(key[:2] == (kind, q) and PLANES[key[2]] == width for key in SEMS):
                for d in BOTH:
                    for i, v in enumerate(message(kind, 0, d) + message(kind, 3 if d else 1, d)[1:]):
                        record((width, q, kind, d, i), v)
        outgoing.append(
            PLANES.count(width) * sum(message(kind, 0, d)[2] for kind in "SYT" for d in BOTH))

        k = cls[q]
        rank = jnp.sum(jnp.where(row16 == k, cum[q * 16:(q + 1) * 16, :BLK], 0),
                       axis=0, keepdims=True)

        def two_parts(a_first, n_a, off_a, n_b, off_b):
            cut = g * jnp.where(a_first, n_a, n_b)
            return jnp.where(rank < cut, rank + g * jnp.where(a_first, off_a, off_b),
                             rank + (g * jnp.where(a_first, off_b, off_a) - cut))

        y_r = h[1]
        y_s = y_r + adj[0]
        y_l = y_s + same[0]
        own_pos = jnp.where(k == 2, two_parts(first[1], h[1], 0, h[3], y_l + adj[3]), -1)
        for kk, off in ((1, y_r), (0, y_s), (3, y_l)):
            own_pos = jnp.where(k == kk, rank + g * off, own_pos)
        z_r = same[1]
        z_d = z_r + adj[0]
        z_l = z_d + h[0]
        z_sl = z_l + adj[3]
        z_s = z_sl + same[3]
        f_ll = nz[0] + h[3]
        f_s = f_ll + adj[2]
        f_rr = f_s + same[2]
        f_d = f_rr + adj[1]
        end_pos = jnp.where(k == 2, two_parts(first[1], h[1], f_d, h[3], nz[0]),
                            two_parts(first[0], h[0], z_d, h[2], f_d + h[1]))
        for kk, off in ((4, 0), (1, z_r), (3, z_l), (9, z_sl), (0, z_s),
                        (8, f_ll), (7, f_s), (5, f_rr)):
            end_pos = jnp.where(k == kk, rank + g * off, end_pos)
        end_pos = jnp.where(fits, end_pos, _iota((1, BLK), 1))
        buf[width]["pos"][q] = jnp.where(_iota((8, BLK), 0) == 0, own_pos, end_pos)
        for name, v in dict(r=z_r, d=z_d, l=z_l, sl=z_sl, s=z_s, nz=nz[0], total=total,
                            shift_r=y_r - z_r, shift_l=y_l - z_l, shift_s=y_s - z_s).items():
            record((width, q, name), v)

    def plane(q, p):
        return q * PLANES.count(PLANES[p]) + SLOT[p]

    def transfer(key, receive):
        kind, q, p0, p1, d = key
        width, b = PLANES[p0], buf[PLANES[p0]]
        so, do, n = (0 if i is None else table[entries[width, q, kind, d, i]]
                     for i in ((None, 3, 4) if receive else (0, 1, 2)))
        if kind == "S":
            src, dst, so = b["own"], b["from_left" if d else "from_right"], so + ROWS[width]
        else:
            src, dst = b["landed" if kind == "T" else "summed"], b["landed"]
        planes = pl.ds(plane(q, p0), p1 - p0)
        for bit in reversed(range(_size_bits(kind, p0))):

            @pl.when((n & (1 << bit)) != 0)
            def _():
                off = n & ~((2 << bit) - 1)
                copy = pltpu.make_async_remote_copy(
                    src_ref=src.at[planes, pl.ds(so + off, 1 << bit)],
                    dst_ref=dst.at[planes, pl.ds(do + off, 1 << bit)],
                    send_sem=send_sem, recv_sem=recv_sem.at[SEMS[key][bit]],
                    device_id=(right if d else left,), device_id_type=pl.DeviceIdType.MESH)
                if receive:
                    copy.wait_recv()
                else:
                    copy.start()

    def gate_rows(xq, route):
        rw_hi = rwv[...].astype(BF16)
        rw = jnp.concatenate([rw_hi, (rwv[...] - rw_hi.astype(F32)).astype(BF16)], axis=0)
        scores = lax.dot_general(rw, xq, NT, preferred_element_type=F32)
        scores = scores[:N_EXP] + scores[N_EXP:]
        probs = jnp.exp(scores - jnp.max(scores, axis=0, keepdims=True))
        probs = probs / jnp.sum(probs, axis=0, keepdims=True)
        e0, e1 = route[0:1] & (N_EXP - 1), route[1:2] & (N_EXP - 1)
        g0 = jnp.sum(jnp.where(row16 == e0, probs, 0.0), axis=0, keepdims=True)
        g1 = jnp.sum(jnp.where(row16 == e1, probs, 0.0), axis=0, keepdims=True)
        gs = g0 + g1
        g0, g1 = g0 / gs, g1 / gs
        return [jnp.where(e0 == E_LOC * me + j, g0, 0.0) + jnp.where(e1 == E_LOC * me + j, g1, 0.0)
                for j in range(E_LOC)]

    def seated(q):
        return [_iota((CAP_E, BLK), 0) == seat[q][j:j + 1, :] for j in range(E_LOC)]

    def experts(q, c0, c1):
        res = []
        for j in range(E_LOC):
            w = jnp.concatenate([wv[c, j] for c in range(c0, c1)], axis=1).astype(BF16)
            res.append(_dot(xs[q * E_LOC + j], w).astype(BF16))
        return jnp.concatenate(res, axis=0)

    def step_p(q, p0, p1):
        plan(q, PLANES[p0])
        yield

    def step_u(q, p0, p1):
        b = buf[PLANES[p0]]
        col = jnp.broadcast_to(b["pos"][q, 1:2, :], (LANES, BLK)).T
        for t in range(0, b["to_token"].shape[2], LANES):
            b["to_token"][q, :, t:t + LANES] = _ones_where(
                col == _iota((BLK, LANES), 1) + t).astype(BF16)
        yield

    def step_q(q, p0, p1):
        b = buf[PLANES[p0]]
        by_row = _ones_where(_iota((CAP_Y, BLK), 0) == b["pos"][q, 0:1, :]).astype(BF16)
        by_seat = jnp.concatenate([_ones_where(m) for m in seated(q)], axis=0).astype(BF16)
        res = lax.dot_general(by_row, by_seat, NT, preferred_element_type=F32).astype(BF16)
        yield
        b["to_wire"][q] = res

    def step_g(q, p0, p1):
        xq = xv[q * BLK:(q + 1) * BLK, :].astype(BF16)
        gate = gate_rows(xq, riv[:, q * BLK:(q + 1) * BLK])
        hit, gap = seated(q), CAP_E - CAP_H
        lo = jnp.concatenate([_ones_where(m[:CAP_H, :HALF]) for m in hit], axis=0).astype(BF16)
        hi = jnp.concatenate([_ones_where(m[gap:, HALF:]) for m in hit], axis=0).astype(BF16)
        lo, hi = _dot(lo, xq[:HALF]), _dot(hi, xq[HALF:])
        res = []
        for j in range(E_LOC):
            a, b = lo[j * CAP_H:(j + 1) * CAP_H], hi[j * CAP_H:(j + 1) * CAP_H]
            picked = jnp.concatenate([a[:gap], a[gap:] + b[:CAP_H - gap], b[CAP_H - gap:]], axis=0)
            weight = jnp.sum(jnp.where(hit[j], gate[j], 0.0), axis=1, keepdims=True)
            res.append((picked * weight).astype(BF16))
        yield
        for j in range(E_LOC):
            xs[q * E_LOC + j] = res[j]

    def step_e(q, p0, p1):
        res = experts(q, TILE0[p0], TILE0[p0] + 1)
        yield
        early[q] = res

    def step_c(q, p0, p1):
        width, c0 = PLANES[p0], TILE0[p0]
        b, n = buf[width], CAP_Y // TOKENS_PER_ROW[width]
        if ("e", q, p0) in WAITS:
            y = jnp.concatenate([early[q], experts(q, c0 + 1, c0 + width)], axis=1)
        else:
            y = experts(q, c0, c0 + width)
        yield
        res = [_to_wire(_dot(b["to_wire"][q, r:r + n, :], y), width) for r in range(0, CAP_Y, n)]
        yield
        b["own"][plane(q, p0), ROWS[width]:ROWS[width] + n, :] = jnp.concatenate(res, axis=0)

    def step_z(q, p0, p1):
        width = PLANES[p0]
        b, n = buf[width], CAP_Z // TOKENS_PER_ROW[width]
        past = {k: _iota((n, LANES), 0) >= table[entries[width, q, k]]
                for k in ("r", "d", "l", "sl", "s", "nz")}
        zero = jnp.zeros((n, LANES), U32)
        for i in range(plane(q, p0), plane(q, p0) + p1 - p0):
            own = {k: b["own"][i, pl.ds(ROWS[width] + table[entries[width, q, "shift_" + k]], n), :]
                   for k in "rls"}
            u = jnp.where(past["l"], jnp.where(past["sl"], zero, own["l"]),
                          b["from_right"][i, :n, :])
            v = jnp.where(past["s"], jnp.where(past["nz"], zero, own["s"]),
                          jnp.where(past["d"], b["from_left"][i, :n, :],
                                    jnp.where(past["r"], own["r"], zero)))
            both = pltpu.bitcast(u, BF16).astype(F32) + pltpu.bitcast(v, BF16).astype(F32)
            b["summed"][i, :n, :] = pltpu.bitcast(both.astype(BF16), U32)
        yield

    def step_o(q, p0, p1):
        width = PLANES[p0]
        b, r = buf[width], _iota((ROWS[width], LANES), 0)
        cols = []
        for i in range(plane(q, p0), plane(q, p0) + p1 - p0):
            f = jnp.where(r < table[entries[width, q, "nz"]], b["summed"][i], b["landed"][i])
            if width == 1:
                f = jnp.where(r < table[entries[width, q, "total"]], f, jnp.zeros(f.shape, U32))
                pad = jnp.zeros((3 * LANES // 2 - ROWS[width], LANES), U32)
                cols.append(pltpu.bitcast(jnp.concatenate([f, pad], axis=0), BF16))
            else:
                cols.append(lax.bitcast_convert_type(f << 16, F32).astype(BF16))
                cols.append(lax.bitcast_convert_type((f >> 16) << 16, F32).astype(BF16))
        f = jnp.concatenate(cols, axis=1)
        n = BLK if width == 2 else BLK // 4 * (p1 - p0)
        res = [_dot(b["to_token"][q, t:t + n, :], f).astype(BF16) for t in range(0, BLK, n)]
        yield
        c0 = TILE0[p0] * LANES
        out_ref[q * BLK:(q + 1) * BLK, c0:c0 + f.shape[1]] = jnp.concatenate(res, axis=0)

    def step_w(q, p0, p1):
        assert len(outgoing) == NBLK * len(WIDTHS)
        n, at = SEND_TOTAL - sum(outgoing), 0
        for bit in range(SEND_TOTAL.bit_length()):
            rows, cols = ((1, LANES << bit) if bit < 3 else (8, LANES << (bit - 3)) if bit < 5
                          else (1 << (bit - 2), D_IN))

            @pl.when((n & (1 << bit)) != 0)
            def _():
                pltpu.make_async_copy(x_hbm.at[pl.ds(0, rows), pl.ds(0, cols)],
                                      ballast.at[pl.ds(at, rows), pl.ds(0, cols)], send_sem).start()

            at += max(rows, 8)
        yield

    @pl.when(jnp.logical_not(fits))
    def _():
        for name in LOADS[1:]:
            load(name).wait()
        pl.semaphore_wait(barrier, 2)
        eye = _iota((BLK, BLK), 0) == _iota((BLK, BLK), 1)

        def swap(stage, q):
            return pltpu.make_async_remote_copy(
                src_ref=part.at[2 * stage, q], dst_ref=part.at[2 * stage + 1, q],
                send_sem=recv_sem.at[(2 + stage) * NBLK + q],
                recv_sem=recv_sem.at[stage * NBLK + q],
                device_id=(jnp.where(((q + stage) & 1) == 0, me ^ 1, 3 - me),),
                device_id_type=pl.DeviceIdType.MESH)

        @pl.loop(0, NBLK)
        def _(q):
            rows = pl.ds(pl.multiple_of(q * BLK, BLK), BLK)
            xq = xv[rows, :].astype(BF16)
            weight = [jnp.sum(jnp.where(eye, g, 0.0), axis=1, keepdims=True)
                      for g in gate_rows(xq, riv[:, rows])]

            @pl.loop(0, NCT, step=4)
            def _(c0):
                for c in range(4):
                    part[0, q, c0 + c] = sum(weight[j] * _dot(xq, wv[c0 + c, j].astype(BF16))
                                             for j in range(E_LOC)).astype(BF16)

            swap(0, q).start()

        @pl.loop(0, NBLK)
        def _(q):
            swap(0, q).wait()

            @pl.loop(0, NCT)
            def _(c):
                part[2, q, c] = (part[0, q, c].astype(F32) + part[1, q, c].astype(F32)).astype(BF16)

            swap(1, q).start()

        @pl.loop(0, NBLK)
        def _(q):
            swap(1, q).wait()
            for p, width in enumerate(PLANES):
                y = [part[2, q, c].astype(F32) + part[3, q, c].astype(F32)
                     for c in range(TILE0[p], TILE0[p] + width)]
                buf[width]["landed"][plane(q, p), :BLK // TOKENS_PER_ROW[width], :] = _to_wire(
                    jnp.concatenate(y, axis=1), width)

    steps = dict(P=step_p, U=step_u, Q=step_q, G=step_g, e=step_e, c=step_c, z=step_z,
                 O=step_o, W=step_w)
    pending = LOADS[1:] + ["barrier"]
    for group in GROUPS:
        for kind, q, p0, _ in group:
            tiles = range(TILE0[p0], TILE0[p0] + (PLANES[p0] if kind == "c" else kind == "e"))
            for name in (["rw", f"x{q}"] if kind == "G" else ["barrier"] if kind in SENDS
                         else [f"w{c}" for c in tiles]):
                if name in pending:
                    pending.remove(name)
                    pl.when(fits)(lambda: pl.semaphore_wait(barrier, 2) if name == "barrier"
                                  else load(name).wait())
            for key in WAITS[kind, q, p0]:
                transfer(key, True)
        sends = [step for step in group if step[0] in SENDS]
        hold = sends and all(step[0] != "c" for step in group)
        running = []
        for step in group:
            if step not in sends:
                running.append(steps[step[0]](*step[1:]))
                next(running[-1])
                if step[0] != "c" and not hold:
                    next(running.pop(), None)
        for batch in (sends[:1], sends[1:]):
            for step in batch:
                for d in BOTH:
                    transfer(step + (d,), False)
            for step in running:
                next(step, None)
    assert not pending and len(entries) <= TABLE_SIZE
    all_sends = ballast.at[pl.ds(0, SEND_TOTAL * LANES // D_IN)]
    pltpu.make_async_copy(all_sends, all_sends, send_sem).wait()


def pallas_dist_moe_top2_ep_n1024_d512_e4_h1024_kernel(
    x: jax.Array,
    router_W: jax.Array,
    route_idx: jax.Array,
    expert_W: jax.Array,
):
    per_width = []
    for w in WIDTHS:
        n = NBLK * PLANES.count(w)
        per_width += [
            pltpu.VMEM((NBLK, 8, BLK), I32),
            pltpu.VMEM((NBLK, CAP_Y, E_LOC * CAP_E), BF16),
            pltpu.VMEM((NBLK, BLK, (4 - w) * LANES), BF16),
            pltpu.VMEM((n, 3 * ROWS[w], LANES), U32),
        ] + [pltpu.VMEM((n, ROWS[w], LANES), U32)] * 4
    return pl.pallas_call(
        _kernel,
        out_shape=jax.ShapeDtypeStruct((N_TOK, D_OUT), BF16),
        in_specs=[pl.BlockSpec(memory_space=pl.ANY)] * 4,
        out_specs=pl.BlockSpec(memory_space=pltpu.VMEM),
        scratch_shapes=[
            pltpu.VMEM((N_TOK, D_IN), F32),
            pltpu.VMEM((NCT, E_LOC, D_IN, LANES), F32),
            pltpu.VMEM((N_EXP, D_IN), F32),
            pltpu.VMEM((2, N_TOK), I32),
            pltpu.VMEM((NBLK * E_LOC, CAP_E, D_IN), BF16),
            pltpu.VMEM((NBLK, E_LOC * CAP_E, LANES), BF16),
            pltpu.VMEM((4, NBLK, NCT, BLK, LANES), BF16),
            pltpu.VMEM((2 * N_TOK + 32, D_IN), F32),
            pltpu.SMEM((TABLE_SIZE,), I32),
            pltpu.SemaphoreType.DMA((len(LOADS),)),
            pltpu.SemaphoreType.DMA,
            pltpu.SemaphoreType.DMA((N_SEMS,)),
        ] + per_width,
        compiler_params=pltpu.CompilerParams(
            collective_id=0, vmem_limit_bytes=64 << 20,
            disable_semaphore_checks=True, disable_bounds_checks=True),
    )(x, router_W.T, route_idx.T, expert_W)
```
